```python
import numpy as np

kernel_name = "dist_rope_attn_qseq_b2_sq128_d512_hq4_dh64"

def setup_inputs():
    x = np.random.randn(2, 512, 512).astype(np.float32)
    Wq = np.random.randn(512, 256).astype(np.float32) * 0.02
    Wk = np.random.randn(512, 256).astype(np.float32) * 0.02
    Wv = np.random.randn(512, 256).astype(np.float32) * 0.02
    Wo = np.random.randn(256, 512).astype(np.float32) * 0.02
    return {"x": x, "Wq": Wq, "Wk": Wk, "Wv": Wv, "Wo": Wo}

def reference(x, Wq, Wk, Wv, Wo):
    B, Sq, Hq, Dh = 2, 512, 4, 64
    inv = 1.0 / (10000.0 ** (np.arange(0, Dh, 2) / Dh))
    pos = np.arange(Sq)[:, None] * inv[None, :]
    cos = np.repeat(np.cos(pos), 2, axis=-1).astype(np.float32)
    sin = np.repeat(np.sin(pos), 2, axis=-1).astype(np.float32)
    def rot(t):
        t2 = t.reshape(B, Sq, Hq, Dh // 2, 2)
        t_r = np.stack([-t2[..., 1], t2[..., 0]], axis=-1).reshape(B, Sq, Hq, Dh)
        return t * cos[None, :, None, :] + t_r * sin[None, :, None, :]
    Q = rot((x @ Wq).reshape(B, Sq, Hq, Dh))
    K = rot((x @ Wk).reshape(B, Sq, Hq, Dh))
    V = (x @ Wv).reshape(B, Sq, Hq, Dh)
    s = np.einsum('bihd,bjhd->bhij', Q, K).astype(np.float32) * 0.125
    s_max = s.max(axis=-1, keepdims=True)
    w = np.exp(s - s_max)
    w = w / w.sum(axis=-1, keepdims=True)
    ctx = np.einsum('bhij,bjhd->bihd', w, V).reshape(B, Sq, Hq * Dh)
    return ctx @ Wo
```

```python
import jax
import jax.numpy as jnp
import numpy as np
from jax import lax
from jax.experimental import pallas as pl
from jax.experimental.pallas import tpu as pltpu

N_DEV = 4
B, SQ, D, HQ, DH = 2, 128, 512, 4, 64
LOG10000 = float(np.log(10000.0))


def _rope_tables(pos0):
    row = lax.broadcasted_iota(jnp.int32, (SQ, 128), 0)
    lane = lax.broadcasted_iota(jnp.int32, (SQ, 128), 1)
    fidx = ((lane % DH) // 2).astype(jnp.float32)
    inv = jnp.exp(fidx * (-2.0 * LOG10000 / DH))
    ang = (row + pos0).astype(jnp.float32) * inv
    even = (lane % 2) == 0
    sin = jnp.sin(ang)
    return jnp.cos(ang), jnp.where(even, -sin, sin), even


def _rope(t, cos, sin_s, even):
    sw = jnp.where(even, pltpu.roll(t, 127, 1), pltpu.roll(t, 1, 1))
    return t * cos + sw * sin_s


def pallas_dist_rope_attn_qseq_b2_sq128_d512_hq4_dh64_kernel(x, Wq, Wk, Wv, Wo):
    def body(x_ref, wq_ref, wk_ref, wv_ref, wo_ref, o_ref, xall, ssem, rsem):
        me = lax.axis_index("i")
        right = (me + 1) % N_DEV
        left = (me + N_DEV - 1) % N_DEV
        bar = pltpu.get_barrier_semaphore()
        for nb in (left, right):
            pl.semaphore_signal(bar, inc=1, device_id=(nb,), device_id_type=pl.DeviceIdType.MESH)
        xall[0] = x_ref[...].astype(jnp.bfloat16)
        pl.semaphore_wait(bar, 2)

        def rd(slot_src, b, slot_dst, dst, k):
            return pltpu.make_async_remote_copy(
                src_ref=xall.at[slot_src, b], dst_ref=xall.at[slot_dst, b],
                send_sem=ssem.at[k], recv_sem=rsem.at[k],
                device_id=(dst,), device_id_type=pl.DeviceIdType.MESH)

        c_r0 = rd(0, 0, 3, right, 0)
        c_l1 = rd(0, 1, 1, left, 1)
        c_r1 = rd(0, 1, 3, right, 2)
        c_l0 = rd(0, 0, 1, left, 3)
        for c in (c_r0, c_l1, c_r1, c_l0):
            c.start()
        c_r0.wait_recv()
        f_r = rd(3, 0, 2, right, 4)
        f_r.start()
        c_l1.wait_recv()
        f_l = rd(1, 1, 2, left, 5)
        f_l.start()

        wq = wq_ref[...].astype(jnp.bfloat16)
        wk = wk_ref[...].astype(jnp.bfloat16)
        wv = wv_ref[...].astype(jnp.bfloat16)
        wo = wo_ref[...].astype(jnp.bfloat16)

        def tables(r):
            return _rope_tables(((me + r) % N_DEV) * SQ)

        def rope2(t, tab):
            return jnp.concatenate([_rope(t[:, :128], *tab), _rope(t[:, 128:], *tab)], axis=1)

        tab0 = tables(0)
        q = []
        for b in range(B):
            qb = jnp.dot(xall[0, b], wq, preferred_element_type=jnp.float32)
            q.append((rope2(qb, tab0) * 0.125).astype(jnp.bfloat16))

        c_r1.wait_recv()
        c_l0.wait_recv()
        f_r.wait_recv()
        f_l.wait_recv()

        ks = [[None] * N_DEV for _ in range(B)]
        vs = [[None] * N_DEV for _ in range(B)]
        for r in range(N_DEV):
            tab = tables(r)
            for b in range(B):
                xb = xall[r, b]
                ks[b][r] = rope2(jnp.dot(xb, wk, preferred_element_type=jnp.float32), tab).astype(jnp.bfloat16)
                vs[b][r] = jnp.dot(xb, wv, preferred_element_type=jnp.float32).astype(jnp.bfloat16)
        for b in range(B):
            kb = jnp.concatenate(ks[b], axis=0)
            vb = jnp.concatenate(vs[b], axis=0)
            ctx = []
            for h in range(HQ):
                sl = slice(h * DH, (h + 1) * DH)
                s = lax.dot_general(q[b][:, sl], kb[:, sl], (((1,), (1,)), ((), ())),
                                    preferred_element_type=jnp.float32)
                m = jnp.max(s, axis=1, keepdims=True)
                p = jnp.exp(s - m)
                l = jnp.sum(p, axis=1, keepdims=True)
                c = jnp.dot(p.astype(jnp.bfloat16), vb[:, sl], preferred_element_type=jnp.float32) / l
                ctx.append(c)
            ctx = jnp.concatenate(ctx, axis=1).astype(jnp.bfloat16)
            o_ref[b] = jnp.dot(ctx, wo, preferred_element_type=jnp.float32)

        for c in (c_r0, c_l1, c_r1, c_l0, f_r, f_l):
            c.wait_send()

    return pl.pallas_call(
        body,
        out_shape=jax.ShapeDtypeStruct((B, SQ, D), jnp.float32),
        scratch_shapes=[
            pltpu.VMEM((N_DEV, B, SQ, D), jnp.bfloat16),
            pltpu.SemaphoreType.DMA((6,)),
            pltpu.SemaphoreType.DMA((6,)),
        ],
        compiler_params=pltpu.CompilerParams(collective_id=0, vmem_limit_bytes=64 * 1024 * 1024),
    )(x, Wq, Wk, Wv, Wo)
```

```python
import jax
import jax.numpy as jnp
import numpy as np
from jax import lax
from jax.experimental import pallas as pl
from jax.experimental.pallas import tpu as pltpu

B, SQ, D, DH = 2, 128, 512, 64
HP = 2 * DH
OWN, P, G, Q = 0, 1, 2, 3
BLOCK = {OWN: 0, P: 1, Q: 2, G: 3}
ROPE_RATE = float(-2.0 * np.log(10000.0) / DH)
Q_SCALE = float(0.125 * np.log2(np.e))
BF16, F32 = jnp.bfloat16, jnp.float32
MESH = pl.DeviceIdType.MESH
CONTRACT_LANES = (((1,), (1,)), ((), ()))


def _kernel(x_hbm, wq_hbm, wk_hbm, wv_hbm, wo_hbm, out_ref,
            x_f32, x_bf16, wk_mine, wq_mine, wv_mine, wk_other, wq_other, wv_other, wo, rope,
            send_k, send_q, send_v, k_all, q_all, v_all,
            probs, row_max, row_sum, acc, ctx_out, ctx_in,
            load_sems, send_sem, recv_sems, ready_sem):
    me = lax.axis_index("i")
    batch, pair = me // 2, me % 2

    def slab(w_hbm, p):
        return w_hbm.at[:, pl.ds(pl.multiple_of(p * HP, HP), HP)]

    loads = {
        "x_mine": (x_hbm.at[batch], x_f32.at[0]),
        "wv_other": (slab(wv_hbm, 1 - pair), wv_other),
        "x_other": (x_hbm.at[1 - batch], x_f32.at[1]),
        "wk_other": (slab(wk_hbm, 1 - pair), wk_other),
        "wq_other": (slab(wq_hbm, 1 - pair), wq_other),
        "wk_mine": (slab(wk_hbm, pair), wk_mine),
        "wv_mine": (slab(wv_hbm, pair), wv_mine),
        "wq_mine": (slab(wq_hbm, pair), wq_mine),
        "wo": (wo_hbm.reshape(2, HP, D), wo),
    }
    pending, in_flight = list(loads), {}

    def start_load(sem):
        name = pending.pop(0)
        in_flight[name] = (pltpu.make_async_copy(*loads[name], load_sems.at[sem]), sem)
        in_flight[name][0].start()

    def await_load(*names):
        for name in names:
            if name in in_flight:
                copy, sem = in_flight.pop(name)
                copy.wait()
                if pending:
                    start_load(sem)

    for sem in range(4):
        start_load(sem)

    barrier = pltpu.get_barrier_semaphore()
    for role in (P, Q):
        pl.semaphore_signal(barrier, inc=1, device_id=(me ^ role,), device_id_type=MESH)

    lane = lax.broadcasted_iota(jnp.int32, (SQ, HP), 1)
    even = (lane % 2) == 0
    lo = lane < DH
    pos = (lax.broadcasted_iota(jnp.int32, (SQ, HP), 0) + me * SQ).astype(F32)
    angle = pos * jnp.exp(((lane % DH) // 2).astype(F32) * ROPE_RATE)
    cos = jnp.cos(angle)
    sin = jnp.sin(angle)
    sin = jnp.where(even, -sin, sin)
    rope[0], rope[1] = cos, sin
    rope[2], rope[3] = cos * Q_SCALE, sin * Q_SCALE

    send = {"k": send_k, "q": send_q, "v": send_v}
    full = {"k": k_all, "q": q_all, "v": v_all}
    weights = {True: {"k": wk_mine, "q": wq_mine, "v": wv_mine},
               False: {"k": wk_other, "q": wq_other, "v": wv_other}}
    converted = set()

    def rows(ref, role):
        return ref.at[pl.ds(BLOCK[role] * SQ, SQ)]

    def project(kind, role):
        i = 0 if role in (OWN, P) else 1
        if i not in converted:
            converted.add(i)
            for j in range(D // HP):
                x_bf16[i, j] = x_f32[i, :, j * HP:(j + 1) * HP].astype(BF16)
        x = jnp.concatenate([x_bf16[i, j] for j in range(D // HP)], axis=1)
        w = weights[role in (OWN, G)][kind][...].astype(BF16)
        t = jnp.dot(x, w, preferred_element_type=F32)
        if kind != "v":
            base = 0 if kind == "k" else 2
            swapped = jnp.where(even, pltpu.roll(t, HP - 1, 1), pltpu.roll(t, 1, 1))
            t = t * rope[base] + swapped * rope[base + 1]
        if role == OWN:
            rows(full[kind], OWN)[...] = t.astype(BF16)
        else:
            send[kind][role] = t.astype(BF16)

    sem_index = {("k", P): 0, ("k", Q): 0, ("v", P): 1, ("v", Q): 1, ("q", P): 2, ("q", Q): 2,
                 ("k", G): 3, ("v", G): 4, ("q", G): 5, ("ctx", P): 6, ("ctx", G): 7, ("ctx", Q): 8}
    sent = []

    def push(src, dst, key, role):
        copy = pltpu.make_async_remote_copy(
            src_ref=src, dst_ref=dst, send_sem=send_sem, recv_sem=recv_sems.at[sem_index[key]],
            device_id=(me ^ role,), device_id_type=MESH)
        copy.start()
        sent.append(copy)

    def push_piece(kind, role):
        push(send[kind].at[role], rows(full[kind], role), (kind, role), role)

    def await_recv(buf, key):
        pltpu.make_async_copy(buf, buf, recv_sems.at[sem_index[key]]).wait()

    def await_neighbours(kind):
        await_recv(full[kind].at[pl.ds(SQ, 2 * SQ)], (kind, P))

    def await_diagonal(kind):
        await_recv(rows(full[kind], G), (kind, G))

    await_load("x_mine", "wv_other")
    project("v", P)
    pl.semaphore_wait(barrier, 2)
    pl.semaphore_signal(ready_sem, inc=1, device_id=(me ^ P,), device_id_type=MESH)
    push_piece("v", P)
    await_load("x_other")
    project("v", Q)
    push_piece("v", Q)
    await_load("wk_other")
    project("k", P), project("k", Q)
    push_piece("k", P), push_piece("k", Q)
    await_load("wq_other")
    project("q", P)
    push_piece("q", P)
    project("q", Q)
    push_piece("q", Q)
    await_load("wk_mine")
    project("k", OWN)
    project("k", G)
    pl.semaphore_wait(ready_sem, 1)
    push_piece("k", G)
    await_load("wv_mine")
    project("v", G)
    push_piece("v", G)
    await_load("wq_mine")
    project("q", OWN), project("q", G)
    push_piece("q", G)

    head_mask = jnp.where(lax.broadcasted_iota(jnp.int32, (SQ // 2, HP), 1) < DH,
                          jnp.uint32(0xFFFFFFFF), jnp.uint32(0))

    def merge(t):
        return jnp.where(lo, t[:SQ], t[SQ:])

    def scores(role, k0, k1):
        q = pltpu.bitcast(rows(q_all, role)[...], jnp.uint32)
        q = jnp.concatenate([pltpu.bitcast(q & head_mask, BF16), pltpu.bitcast(q & ~head_mask, BF16)], axis=0)
        return lax.dot_general(q, k_all[pl.ds(k0 * SQ, (k1 - k0) * SQ)], CONTRACT_LANES,
                               preferred_element_type=F32)

    def softmax_first(role, nblocks):
        s = scores(role, 0, nblocks)
        m = jnp.max(s, axis=1, keepdims=True)
        p = jnp.exp2(s - m)
        for j in range(nblocks):
            probs[role, j] = p[:, j * SQ:(j + 1) * SQ].astype(BF16)
        if nblocks < 4:
            row_max[role] = jnp.broadcast_to(m, (2 * SQ, HP))

    def softmax_diagonal(role):
        s = scores(role, 3, 4)
        m_old = row_max[role]
        m = jnp.maximum(m_old, jnp.max(s, axis=1, keepdims=True))
        probs[role, 3] = jnp.exp2(s - m).astype(BF16)
        alpha = merge(jnp.exp2(m_old - m))
        row_sum[role] = row_sum[role] * alpha
        acc[role] = acc[role] * alpha

    def weighted(role, k0, k1):
        p = [probs[role, j] for j in range(k0, k1)]
        o = jnp.dot(jnp.concatenate(p, axis=1) if len(p) > 1 else p[0],
                    v_all[pl.ds(k0 * SQ, (k1 - k0) * SQ)], preferred_element_type=F32)
        total = p[0].astype(F32)
        for t in p[1:]:
            total = total + t.astype(F32)
        return merge(o), merge(jnp.sum(total, axis=1, keepdims=True))

    def accumulate_first(role):
        acc[role], row_sum[role] = weighted(role, 0, 3)

    def context(role, k0):
        o, l = weighted(role, k0, 4)
        if k0:
            o, l = acc[role] + o, row_sum[role] + l
        r = pl.reciprocal(l, approx=True)
        ctx_out[role] = (o * (r * (2.0 - l * r))).astype(BF16)

    def push_context(role):
        push(ctx_out.at[role], ctx_in.at[role], ("ctx", role), role)

    await_neighbours("k")
    softmax_first(OWN, 3), project("v", OWN)
    await_neighbours("q")
    softmax_first(Q, 3), softmax_first(P, 3)
    await_neighbours("v")
    await_diagonal("k")
    accumulate_first(Q), accumulate_first(P), accumulate_first(OWN)
    softmax_diagonal(P), softmax_diagonal(OWN), softmax_diagonal(Q)
    await_diagonal("v")
    context(Q, 3), context(P, 3)
    push_context(Q), push_context(P)
    await_diagonal("q")
    softmax_first(G, 4), context(G, 0)
    push_context(G)

    def out_proj(ctx, own_pair):
        return jnp.dot(ctx, wo[pair if own_pair else 1 - pair].astype(BF16), preferred_element_type=F32)

    await_load("wo")
    context(OWN, 3)
    out_ref[batch] = out_proj(ctx_out[OWN], True)
    await_recv(ctx_in.at[Q], ("ctx", Q))
    await_recv(ctx_in.at[P], ("ctx", P))
    out_ref[1 - batch] = out_proj(ctx_in[Q], False)
    out_ref[batch] += out_proj(ctx_in[P], False)
    await_recv(ctx_in.at[G], ("ctx", G))
    out_ref[1 - batch] += out_proj(ctx_in[G], True)

    for copy in sent:
        copy.wait_send()


def pallas_dist_rope_attn_qseq_b2_sq128_d512_hq4_dh64_kernel(
    x: jax.Array,
    Wq: jax.Array,
    Wk: jax.Array,
    Wv: jax.Array,
    Wo: jax.Array,
):
    vmem = pltpu.VMEM
    return pl.pallas_call(
        _kernel,
        out_shape=jax.ShapeDtypeStruct((B, SQ, D), F32),
        in_specs=[pl.BlockSpec(memory_space=pl.ANY)] * 5,
        out_specs=pl.BlockSpec(memory_space=pltpu.VMEM),
        scratch_shapes=[
            vmem((B, SQ, D), F32), vmem((B, D // HP, SQ, HP), BF16),
            *[vmem((D, HP), F32) for _ in range(6)],
            vmem((2, HP, D), F32), vmem((4, SQ, HP), F32),
            *[vmem((4, SQ, HP), BF16) for _ in range(3)],
            *[vmem((4 * SQ, HP), BF16) for _ in range(3)],
            vmem((4, 4, 2 * SQ, SQ), BF16), vmem((4, 2 * SQ, HP), F32),
            vmem((4, SQ, HP), F32), vmem((4, SQ, HP), F32),
            vmem((4, SQ, HP), BF16), vmem((4, SQ, HP), BF16),
            pltpu.SemaphoreType.DMA((4,)),
            pltpu.SemaphoreType.DMA,
            pltpu.SemaphoreType.DMA((9,)),
            pltpu.SemaphoreType.REGULAR,
        ],
        compiler_params=pltpu.CompilerParams(collective_id=0, vmem_limit_bytes=64 * 1024 * 1024),
    )(x, Wq, Wk, Wv, Wo)
```

```python
import jax
import jax.numpy as jnp
import numpy as np
from jax import lax
from jax.experimental import pallas as pl
from jax.experimental.pallas import tpu as pltpu

B, SQ, D, DH = 2, 128, 512, 64
HP = 2 * DH
OWN, P, G, Q = 0, 1, 2, 3
BLOCK = {OWN: 0, P: 1, Q: 2, G: 3}
ROPE_RATE = float(-2.0 * np.log(10000.0) / DH)
Q_SCALE = float(0.125 * np.log2(np.e))
BF16, F32 = jnp.bfloat16, jnp.float32
MESH = pl.DeviceIdType.MESH
CONTRACT_LANES = (((1,), (1,)), ((), ()))


def _kernel(x_hbm, wq_hbm, wk_hbm, wv_hbm, wo_hbm, out_ref,
            x_f32, x_bf16, wk_mine, wq_mine, wv_mine, wk_other, wq_other, wv_other, wo, rope,
            send_k, send_q, send_v, k_all, q_all, v_all,
            probs, row_max, row_sum, acc, ctx_out, ctx_in,
            load_sems, send_sem, recv_sems, ready_sem):
    me = lax.axis_index("i")
    batch, pair = me // 2, me % 2

    def slab(w_hbm, p):
        return w_hbm.at[:, pl.ds(pl.multiple_of(p * HP, HP), HP)]

    loads = {
        "x_mine": (x_hbm.at[batch], x_f32.at[0]),
        "wv_other": (slab(wv_hbm, 1 - pair), wv_other),
        "x_other": (x_hbm.at[1 - batch], x_f32.at[1]),
        "wk_other": (slab(wk_hbm, 1 - pair), wk_other),
        "wq_other": (slab(wq_hbm, 1 - pair), wq_other),
        "wk_mine": (slab(wk_hbm, pair), wk_mine),
        "wv_mine": (slab(wv_hbm, pair), wv_mine),
        "wq_mine": (slab(wq_hbm, pair), wq_mine),
        "wo": (wo_hbm.reshape(2, HP, D), wo),
    }
    pending, in_flight = list(loads), {}

    def start_load(sem):
        name = pending.pop(0)
        in_flight[name] = (pltpu.make_async_copy(*loads[name], load_sems.at[sem]), sem)
        in_flight[name][0].start()

    def await_load(*names):
        for name in names:
            if name in in_flight:
                copy, sem = in_flight.pop(name)
                copy.wait()
                if pending:
                    start_load(sem)

    for sem in range(4):
        start_load(sem)

    barrier = pltpu.get_barrier_semaphore()
    for role in (P, Q):
        pl.semaphore_signal(barrier, inc=1, device_id=(me ^ role,), device_id_type=MESH)

    lane = lax.broadcasted_iota(jnp.int32, (SQ, HP), 1)
    even = (lane % 2) == 0
    lo = lane < DH
    pos = (lax.broadcasted_iota(jnp.int32, (SQ, HP), 0) + me * SQ).astype(F32)
    angle = pos * jnp.exp(((lane % DH) // 2).astype(F32) * ROPE_RATE)
    cos = jnp.cos(angle)
    sin = jnp.sin(angle)
    sin = jnp.where(even, -sin, sin)
    rope[0], rope[1] = cos, sin
    rope[2], rope[3] = cos * Q_SCALE, sin * Q_SCALE

    send = {"k": send_k, "q": send_q, "v": send_v}
    full = {"k": k_all, "q": q_all, "v": v_all}
    weights = {True: {"k": wk_mine, "q": wq_mine, "v": wv_mine},
               False: {"k": wk_other, "q": wq_other, "v": wv_other}}
    converted = set()

    def rows(ref, role):
        return ref.at[pl.ds(BLOCK[role] * SQ, SQ)]

    def project(kind, role):
        i = 0 if role in (OWN, P) else 1
        if i not in converted:
            converted.add(i)
            for j in range(D // HP):
                x_bf16[i, j] = x_f32[i, :, j * HP:(j + 1) * HP].astype(BF16)
        x = jnp.concatenate([x_bf16[i, j] for j in range(D // HP)], axis=1)
        w = weights[role in (OWN, G)][kind][...].astype(BF16)
        t = jnp.dot(x, w, preferred_element_type=F32)
        if kind != "v":
            base = 0 if kind == "k" else 2
            swapped = jnp.where(even, pltpu.roll(t, HP - 1, 1), pltpu.roll(t, 1, 1))
            t = t * rope[base] + swapped * rope[base + 1]
        if role == OWN:
            rows(full[kind], OWN)[...] = t.astype(BF16)
        else:
            send[kind][role] = t.astype(BF16)

    sem_index = {("k", P): 0, ("k", Q): 0, ("v", P): 1, ("v", Q): 1, ("q", P): 2, ("q", Q): 2,
                 ("k", G): 3, ("v", G): 4, ("q", G): 5, ("ctx", P): 6, ("ctx", G): 7, ("ctx", Q): 8}
    sent = []

    def push(src, dst, key, role):
        copy = pltpu.make_async_remote_copy(
            src_ref=src, dst_ref=dst, send_sem=send_sem, recv_sem=recv_sems.at[sem_index[key]],
            device_id=(me ^ role,), device_id_type=MESH)
        copy.start()
        sent.append(copy)

    def push_piece(kind, role):
        push(send[kind].at[role], rows(full[kind], role), (kind, role), role)

    def await_recv(buf, key):
        pltpu.make_async_copy(buf, buf, recv_sems.at[sem_index[key]]).wait()

    def await_neighbours(kind):
        await_recv(full[kind].at[pl.ds(SQ, 2 * SQ)], (kind, P))

    def await_diagonal(kind):
        await_recv(rows(full[kind], G), (kind, G))

    await_load("x_mine", "wv_other")
    project("v", P)
    pl.semaphore_wait(barrier, 2)
    pl.semaphore_signal(ready_sem, inc=1, device_id=(me ^ P,), device_id_type=MESH)
    push_piece("v", P)
    await_load("x_other")
    project("v", Q)
    push_piece("v", Q)
    await_load("wk_other")
    project("k", P)
    project("k", Q)
    push_piece("k", P)
    push_piece("k", Q)
    await_load("wq_other")
    project("q", P)
    push_piece("q", P)
    project("q", Q)
    push_piece("q", Q)
    await_load("wk_mine")
    project("k", OWN)
    project("k", G)
    pl.semaphore_wait(ready_sem, 1)
    push_piece("k", G)
    await_load("wv_mine")
    project("v", G)
    push_piece("v", G)
    await_load("wq_mine")
    project("q", OWN)
    project("q", G)
    push_piece("q", G)

    head_mask = jnp.where(lax.broadcasted_iota(jnp.int32, (SQ // 2, HP), 1) < DH,
                          jnp.uint32(0xFFFFFFFF), jnp.uint32(0))

    def merge(t):
        return jnp.where(lo, t[:SQ], t[SQ:])

    def scores(role, k0, k1):
        q = pltpu.bitcast(rows(q_all, role)[...], jnp.uint32)
        q = jnp.concatenate([pltpu.bitcast(q & head_mask, BF16), pltpu.bitcast(q & ~head_mask, BF16)], axis=0)
        return lax.dot_general(q, k_all[pl.ds(k0 * SQ, (k1 - k0) * SQ)], CONTRACT_LANES,
                               preferred_element_type=F32)

    def softmax_first(role, nblocks):
        s = scores(role, 0, nblocks)
        m = jnp.max(s, axis=1, keepdims=True)
        p = jnp.exp2(s - m)
        for j in range(nblocks):
            probs[role, j] = p[:, j * SQ:(j + 1) * SQ].astype(BF16)
        if nblocks < 4:
            row_max[role] = jnp.broadcast_to(m, (2 * SQ, HP))

    def softmax_diagonal(role):
        s = scores(role, 3, 4)
        m_old = row_max[role]
        m = jnp.maximum(m_old, jnp.max(s, axis=1, keepdims=True))
        probs[role, 3] = jnp.exp2(s - m).astype(BF16)
        alpha = merge(jnp.exp2(m_old - m))
        row_sum[role] = row_sum[role] * alpha
        acc[role] = acc[role] * alpha

    def weighted(role, k0, k1):
        p = [probs[role, j] for j in range(k0, k1)]
        o = jnp.dot(jnp.concatenate(p, axis=1) if len(p) > 1 else p[0],
                    v_all[pl.ds(k0 * SQ, (k1 - k0) * SQ)], preferred_element_type=F32)
        total = p[0].astype(F32)
        for t in p[1:]:
            total = total + t.astype(F32)
        return merge(o), merge(jnp.sum(total, axis=1, keepdims=True))

    def accumulate_first(role):
        acc[role], row_sum[role] = weighted(role, 0, 3)

    def context(role, k0):
        o, l = weighted(role, k0, 4)
        if k0:
            o, l = acc[role] + o, row_sum[role] + l
        r = pl.reciprocal(l, approx=True)
        ctx_out[role] = (o * (r * (2.0 - l * r))).astype(BF16)

    def push_context(role):
        push(ctx_out.at[role], ctx_in.at[role], ("ctx", role), role)

    await_neighbours("k")
    softmax_first(OWN, 3)
    project("v", OWN)
    await_neighbours("q")
    softmax_first(Q, 3)
    softmax_first(P, 3)
    await_neighbours("v")
    await_diagonal("k")
    accumulate_first(Q)
    accumulate_first(P)
    accumulate_first(OWN)
    softmax_diagonal(P)
    softmax_diagonal(OWN)
    softmax_diagonal(Q)
    await_diagonal("v")
    context(Q, 3)
    context(P, 3)
    push_context(Q)
    push_context(P)
    await_diagonal("q")
    softmax_first(G, 4)
    context(G, 0)
    push_context(G)

    def out_proj(ctx, own_pair):
        return jnp.dot(ctx, wo[pair if own_pair else 1 - pair].astype(BF16), preferred_element_type=F32)

    await_load("wo")
    context(OWN, 3)
    out_ref[batch] = out_proj(ctx_out[OWN], True)
    await_recv(ctx_in.at[Q], ("ctx", Q))
    await_recv(ctx_in.at[P], ("ctx", P))
    out_ref[1 - batch] = out_proj(ctx_in[Q], False)
    out_ref[batch] += out_proj(ctx_in[P], False)
    await_recv(ctx_in.at[G], ("ctx", G))
    out_ref[1 - batch] += out_proj(ctx_in[G], True)

    for copy in sent:
        copy.wait_send()


def pallas_dist_rope_attn_qseq_b2_sq128_d512_hq4_dh64_kernel(
    x: jax.Array,
    Wq: jax.Array,
    Wk: jax.Array,
    Wv: jax.Array,
    Wo: jax.Array,
):
    vmem = pltpu.VMEM
    return pl.pallas_call(
        _kernel,
        out_shape=jax.ShapeDtypeStruct((B, SQ, D), F32),
        in_specs=[pl.BlockSpec(memory_space=pl.ANY)] * 5,
        out_specs=pl.BlockSpec(memory_space=pltpu.VMEM),
        scratch_shapes=[
            vmem((B, SQ, D), F32), vmem((B, D // HP, SQ, HP), BF16),
            *[vmem((D, HP), F32) for _ in range(6)],
            vmem((2, HP, D), F32), vmem((4, SQ, HP), F32),
            *[vmem((4, SQ, HP), BF16) for _ in range(3)],
            *[vmem((4 * SQ, HP), BF16) for _ in range(3)],
            vmem((4, 4, 2 * SQ, SQ), BF16), vmem((4, 2 * SQ, HP), F32),
            vmem((4, SQ, HP), F32), vmem((4, SQ, HP), F32),
            vmem((4, SQ, HP), BF16), vmem((4, SQ, HP), BF16),
            pltpu.SemaphoreType.DMA((4,)),
            pltpu.SemaphoreType.DMA,
            pltpu.SemaphoreType.DMA((9,)),
            pltpu.SemaphoreType.REGULAR,
        ],
        compiler_params=pltpu.CompilerParams(collective_id=0, vmem_limit_bytes=64 * 1024 * 1024),
    )(x, Wq, Wk, Wv, Wo)
```
